```python
import numpy as np

kernel_name = "dist_mean_ax0_shard0_i_m1024_n512"

def setup_inputs():
    return {"x": np.random.randn(4096, 512).astype(np.float32)}

def reference(x: np.ndarray) -> np.ndarray:
    return np.mean(x, axis=0, keepdims=True)
```

```python
import jax
import jax.numpy as jnp
from jax import lax
from jax.experimental import pallas as pl
from jax.experimental.pallas import tpu as pltpu

N_DEV = 4
N_CHUNKS = 8


def pallas_dist_mean_ax0_shard0_i_m1024_n512_kernel(
    x: jax.Array,
):
    m, n = x.shape
    rows = m // N_CHUNKS
    inv_count = 1.0 / (m * N_DEV)

    def body(x_hbm, out_ref, xbuf, part, load_sems, send_sems, recv_sems):
        my = lax.axis_index("i")

        barrier = pltpu.get_barrier_semaphore()
        for d in range(1, N_DEV):
            pl.semaphore_signal(
                barrier, inc=1,
                device_id=((my + d) % N_DEV,),
                device_id_type=pl.DeviceIdType.MESH,
            )

        loads = []
        for c in range(N_CHUNKS):
            cp = pltpu.make_async_copy(
                x_hbm.at[pl.ds(c * rows, rows)],
                xbuf.at[pl.ds(c * rows, rows)],
                load_sems.at[c],
            )
            cp.start()
            loads.append(cp)

        acc = jnp.zeros((8, n), jnp.float32)
        for c in range(N_CHUNKS):
            loads[c].wait()
            blk = xbuf[pl.ds(c * rows, rows), :]
            acc = acc + jnp.sum(blk.reshape(rows // 8, 8, n), axis=0)
        part[0] = jnp.sum(acc, axis=0, keepdims=True)

        pl.semaphore_wait(barrier, N_DEV - 1)

        rdmas = []
        for d in range(1, N_DEV):
            r = pltpu.make_async_remote_copy(
                src_ref=part.at[0],
                dst_ref=part.at[d],
                send_sem=send_sems.at[d - 1],
                recv_sem=recv_sems.at[d - 1],
                device_id=((my + d) % N_DEV,),
                device_id_type=pl.DeviceIdType.MESH,
            )
            r.start()
            rdmas.append(r)
        for r in rdmas:
            r.wait_recv()
        out_ref[...] = (part[0] + part[1] + part[2] + part[3]) * inv_count
        for r in rdmas:
            r.wait_send()

    return pl.pallas_call(
        body,
        out_shape=jax.ShapeDtypeStruct((1, n), jnp.float32),
        in_specs=[pl.BlockSpec(memory_space=pl.ANY)],
        out_specs=pl.BlockSpec(memory_space=pltpu.VMEM),
        scratch_shapes=[
            pltpu.VMEM((m, n), jnp.float32),
            pltpu.VMEM((N_DEV, 1, n), jnp.float32),
            pltpu.SemaphoreType.DMA((N_CHUNKS,)),
            pltpu.SemaphoreType.DMA((N_DEV - 1,)),
            pltpu.SemaphoreType.DMA((N_DEV - 1,)),
        ],
        compiler_params=pltpu.CompilerParams(collective_id=0),
    )(x)
```

```python
import jax
import jax.numpy as jnp
from jax import lax
from jax.experimental import pallas as pl
from jax.experimental.pallas import tpu as pltpu

N_DEV = 4
LANES = 128
SUBLANES = 8
RAW_ROWS = 32
TAIL_ROWS = 32


def _tree_sum(vals):
    vals = list(vals)
    while len(vals) > 1:
        nxt = [vals[i] + vals[i + 1] for i in range(0, len(vals) - 1, 2)]
        if len(vals) % 2:
            nxt.append(vals[-1])
        vals = nxt
    return vals[0]


def _fold_rows(ref, row0, nrows, n_acc=3):
    accs = [None] * n_acc
    for t in range(nrows // SUBLANES):
        v = ref[pl.ds(row0 + SUBLANES * t, SUBLANES), :]
        a = t % n_acc
        accs[a] = v if accs[a] is None else accs[a] + v
    return _tree_sum(a for a in accs if a is not None)


def _main_chunks(rows):
    chunks = []
    size = 512
    while rows > 0:
        while size > rows:
            size //= 2
        size = max(size, SUBLANES)
        chunks.append(size)
        rows -= size
        size = max(size // 2, SUBLANES)
    return chunks


def _compiler_params():
    try:
        return pltpu.CompilerParams(collective_id=0, disable_semaphore_checks=True)
    except TypeError:
        return pltpu.CompilerParams(collective_id=0)


def pallas_dist_mean_ax0_shard0_i_m1024_n512_kernel(
    x: jax.Array,
):
    m, n = x.shape
    n_groups = n // LANES
    tail0 = m - RAW_ROWS - TAIL_ROWS
    raw0 = m - RAW_ROWS
    chunks = _main_chunks(tail0)
    starts = [sum(chunks[:c]) for c in range(len(chunks))]
    scale = 1.0 / (m * N_DEV)

    n_loads = len(chunks) + n_groups + 1
    sem_left, sem_right, sem_raw = n_groups, n_groups + 1, n_groups + 2
    n_msgs = n_groups + 3

    def body(x_hbm, out_ref, xbuf, rawbuf, part, full, load_sems, send_sems, recv_sems):
        def load(rows, cols, sem):
            cp = pltpu.make_async_copy(
                x_hbm.at[rows, cols], xbuf.at[rows, cols], load_sems.at[sem])
            cp.start()
            return cp

        all_cols = pl.ds(0, n)
        main_loads = [
            load(pl.ds(starts[c], r), all_cols, c) for c, r in enumerate(chunks)
        ]
        tail_loads = [
            load(pl.ds(tail0, TAIL_ROWS), pl.ds(g * LANES, LANES), len(chunks) + g)
            for g in range(n_groups)
        ]
        raw_load = load(pl.ds(raw0, RAW_ROWS), all_cols, n_loads - 1)

        my = lax.axis_index("i")
        peer = {d: lax.rem(my + d, N_DEV) for d in range(1, N_DEV)}
        barrier = pltpu.get_barrier_semaphore()
        for d in (2, 1, 3):
            pl.semaphore_signal(
                barrier, inc=1, device_id=(peer[d],),
                device_id_type=pl.DeviceIdType.MESH)
        pl.semaphore_wait(barrier, N_DEV - 1)

        def send(src, dst, sem, d):
            cp = pltpu.make_async_remote_copy(
                src_ref=src, dst_ref=dst,
                send_sem=send_sems.at[sem], recv_sem=recv_sems.at[sem],
                device_id=(peer[d],), device_id_type=pl.DeviceIdType.MESH)
            cp.start()
            return cp

        raw_msg = send(x_hbm.at[pl.ds(raw0, RAW_ROWS)], rawbuf, sem_raw, 2)

        acc = None
        for c, r in enumerate(chunks):
            main_loads[c].wait()
            s = _fold_rows(xbuf, starts[c], r)
            acc = s if acc is None else acc + s

        diag_msgs = []
        for g in range(n_groups):
            cols = pl.ds(g * LANES, LANES)
            tail_loads[g].wait()
            t = _tree_sum(
                xbuf[pl.ds(tail0 + SUBLANES * i, SUBLANES), cols]
                for i in range(TAIL_ROWS // SUBLANES))
            t = t + acc[:, g * LANES:(g + 1) * LANES]
            part[0, :, cols] = jnp.sum(t, axis=0, keepdims=True) * scale
            diag_msgs.append(send(part.at[0, :, cols], part.at[2, :, cols], g, 2))

        raw_load.wait()
        e = _fold_rows(xbuf, raw0, RAW_ROWS)
        full[...] = part[0] + jnp.sum(e, axis=0, keepdims=True) * scale
        nbr_msgs = [
            send(full, part.at[1], sem_right, 1),
            send(full, part.at[3], sem_left, 3),
        ]

        for cp in diag_msgs + nbr_msgs + [raw_msg]:
            cp.wait_send()

        for cp in nbr_msgs:
            cp.wait_recv()
        res = full[...] + part[1] + part[3]
        raw_msg.wait_recv()
        r = _fold_rows(rawbuf, 0, RAW_ROWS)
        full[...] = res + jnp.sum(r, axis=0, keepdims=True) * scale
        res = full[...]
        for cp in diag_msgs:
            cp.wait_recv()
        out_ref[...] = res + part[2]

    return pl.pallas_call(
        body,
        out_shape=jax.ShapeDtypeStruct((1, n), jnp.float32),
        in_specs=[pl.BlockSpec(memory_space=pl.ANY)],
        out_specs=pl.BlockSpec(memory_space=pltpu.VMEM),
        scratch_shapes=[
            pltpu.VMEM((m, n), jnp.float32),
            pltpu.VMEM((RAW_ROWS, n), jnp.float32),
            pltpu.VMEM((N_DEV, 1, n), jnp.float32),
            pltpu.VMEM((1, n), jnp.float32),
            pltpu.SemaphoreType.DMA((n_loads,)),
            pltpu.SemaphoreType.DMA((n_msgs,)),
            pltpu.SemaphoreType.DMA((n_msgs,)),
        ],
        compiler_params=_compiler_params(),
    )(x)
```

```python
import jax
import jax.numpy as jnp
from jax import lax
from jax.experimental import pallas as pl
from jax.experimental.pallas import tpu as pltpu

N_DEV = 4
LANES = 128
SUBLANES = 8
RAW_ROWS = 24
TAIL_ROWS = 48


def _tree_sum(vals):
    vals = list(vals)
    while len(vals) > 1:
        nxt = [vals[i] + vals[i + 1] for i in range(0, len(vals) - 1, 2)]
        if len(vals) % 2:
            nxt.append(vals[-1])
        vals = nxt
    return vals[0]


def _fold_rows(ref, row0, nrows, n_acc=3):
    accs = [None] * n_acc
    for t in range(nrows // SUBLANES):
        v = ref[pl.ds(row0 + SUBLANES * t, SUBLANES), :]
        a = t % n_acc
        accs[a] = v if accs[a] is None else accs[a] + v
    return _tree_sum(a for a in accs if a is not None)


def _main_chunks(rows):
    chunks = []
    for size in (512, 256, 128):
        if rows > size:
            chunks.append(size)
            rows -= size
    chunks.append(rows)
    return chunks


def _compiler_params():
    try:
        return pltpu.CompilerParams(collective_id=0, disable_semaphore_checks=True)
    except TypeError:
        return pltpu.CompilerParams(collective_id=0)


def pallas_dist_mean_ax0_shard0_i_m1024_n512_kernel(
    x: jax.Array,
):
    m, n = x.shape
    n_groups = n // LANES
    tail0 = m - RAW_ROWS - TAIL_ROWS
    raw0 = m - RAW_ROWS
    chunks = _main_chunks(tail0)
    starts = [sum(chunks[:c]) for c in range(len(chunks))]
    scale = 1.0 / (m * N_DEV)

    n_loads = len(chunks) + n_groups + 1
    sem_left, sem_right, sem_raw = n_groups, n_groups + 1, n_groups + 2
    n_msgs = n_groups + 3

    def body(x_hbm, out_ref, xbuf, rawbuf, part, full, load_sems, send_sems, recv_sems):
        def load(rows, cols, sem):
            cp = pltpu.make_async_copy(
                x_hbm.at[rows, cols], xbuf.at[rows, cols], load_sems.at[sem])
            cp.start()
            return cp

        all_cols = pl.ds(0, n)
        main_loads = [
            load(pl.ds(starts[c], r), all_cols, c) for c, r in enumerate(chunks)
        ]
        tail_loads = [
            load(pl.ds(tail0, TAIL_ROWS), pl.ds(g * LANES, LANES), len(chunks) + g)
            for g in range(n_groups)
        ]
        raw_load = load(pl.ds(raw0, RAW_ROWS), all_cols, n_loads - 1)

        my = lax.axis_index("i")
        peer = {d: lax.rem(my + d, N_DEV) for d in range(1, N_DEV)}
        barrier = pltpu.get_barrier_semaphore()
        for d in (2, 1, 3):
            pl.semaphore_signal(
                barrier, inc=1, device_id=(peer[d],),
                device_id_type=pl.DeviceIdType.MESH)
        pl.semaphore_wait(barrier, N_DEV - 1)

        def send(src, dst, sem, d):
            cp = pltpu.make_async_remote_copy(
                src_ref=src, dst_ref=dst,
                send_sem=send_sems.at[sem], recv_sem=recv_sems.at[sem],
                device_id=(peer[d],), device_id_type=pl.DeviceIdType.MESH)
            cp.start()
            return cp

        raw_msg = send(x_hbm.at[pl.ds(raw0, RAW_ROWS)], rawbuf, sem_raw, 2)

        acc = None
        for c, r in enumerate(chunks):
            main_loads[c].wait()
            s = _fold_rows(xbuf, starts[c], r)
            acc = s if acc is None else acc + s

        diag_msgs = []
        for g in range(n_groups):
            cols = pl.ds(g * LANES, LANES)
            tail_loads[g].wait()
            t = _tree_sum(
                xbuf[pl.ds(tail0 + SUBLANES * i, SUBLANES), cols]
                for i in range(TAIL_ROWS // SUBLANES))
            t = t + acc[:, g * LANES:(g + 1) * LANES]
            part[0, :, cols] = jnp.sum(t, axis=0, keepdims=True) * scale
            diag_msgs.append(send(part.at[0, :, cols], part.at[2, :, cols], g, 2))

        raw_load.wait()
        e = _fold_rows(xbuf, raw0, RAW_ROWS)
        full[...] = part[0] + jnp.sum(e, axis=0, keepdims=True) * scale
        nbr_msgs = [
            send(full, part.at[1], sem_right, 1),
            send(full, part.at[3], sem_left, 3),
        ]

        for cp in diag_msgs + nbr_msgs + [raw_msg]:
            cp.wait_send()

        for cp in nbr_msgs:
            cp.wait_recv()
        res = full[...] + part[1] + part[3]
        raw_msg.wait_recv()
        r = _fold_rows(rawbuf, 0, RAW_ROWS)
        full[...] = res + jnp.sum(r, axis=0, keepdims=True) * scale
        res = full[...]
        for cp in diag_msgs:
            cp.wait_recv()
        out_ref[...] = res + part[2]

    return pl.pallas_call(
        body,
        out_shape=jax.ShapeDtypeStruct((1, n), jnp.float32),
        in_specs=[pl.BlockSpec(memory_space=pl.ANY)],
        out_specs=pl.BlockSpec(memory_space=pltpu.VMEM),
        scratch_shapes=[
            pltpu.VMEM((m, n), jnp.float32),
            pltpu.VMEM((RAW_ROWS, n), jnp.float32),
            pltpu.VMEM((N_DEV, 1, n), jnp.float32),
            pltpu.VMEM((1, n), jnp.float32),
            pltpu.SemaphoreType.DMA((n_loads,)),
            pltpu.SemaphoreType.DMA((n_msgs,)),
            pltpu.SemaphoreType.DMA((n_msgs,)),
        ],
        compiler_params=_compiler_params(),
    )(x)
```
